```python
import numpy as np

kernel_name = "dist_sparse_attn_blocksparse_qseq_kvseq_b2_sq256_skv256_hq4_dh64"

def setup_inputs():
    x = np.random.randn(2, 1024, 512).astype(np.float32)
    Wq = np.random.randn(512, 256).astype(np.float32) * 0.02
    K_ext = np.random.randn(2, 1024, 4, 64).astype(np.float32)
    V_ext = np.random.randn(2, 1024, 4, 64).astype(np.float32)
    Wo = np.random.randn(256, 512).astype(np.float32) * 0.02
    return {"x": x, "Wq": Wq, "K_ext": K_ext, "V_ext": V_ext, "Wo": Wo}

def reference(x, Wq, K_ext, V_ext, Wo):
    B, Sq, Skv, Hq, Dh = 2, 1024, 1024, 4, 64
    Q = (x @ Wq).reshape(B, Sq, Hq, Dh)
    qb = (np.arange(Sq) // 64)[:, None]
    kb = (np.arange(Skv) // 64)[None, :]
    mask = (qb == kb) | (kb == 0) | ((qb + kb) % 3 == 0)
    scores = np.einsum('bihd,bjhd->bhij', Q, K_ext).astype(np.float32) * 0.125
    scores = np.where(mask[None, None, :, :], scores, -1e9)
    scores_max = scores.max(axis=-1, keepdims=True)
    w = np.exp(scores - scores_max)
    row_keep = mask.any(axis=1)
    w_sum = np.where(row_keep[None, None, :, None], w.sum(axis=-1, keepdims=True), 1.0)
    w = w / w_sum
    w = np.where(row_keep[None, None, :, None], w, 0.0)
    ctx = np.einsum('bhij,bjhd->bihd', w, V_ext).reshape(B, Sq, Hq * Dh)
    return ctx @ Wo
```

```python
import functools

import jax
import jax.numpy as jnp
from jax import lax
from jax.experimental import pallas as pl
from jax.experimental.pallas import tpu as pltpu

F32 = jnp.float32
BF16 = jnp.bfloat16
U32 = jnp.uint32
MESH = pl.DeviceIdType.MESH
NEG = -1e30
NT = (((1,), (1,)), ((), ()))
QSCALE = 0.125 * 1.4426950408889634


EARLY_Q = (
    ((1, 0), (1, 1), (1, 2), (1, 3)),
    ((1, 0), (1, 1), (1, 2), (1, 3)),
    ((1, 0), (1, 1)),
    (),
)
LINK_Q = (
    ((2, 0), (2, 1), (2, 2), (2, 3), (3, 0), (3, 1), (3, 2), (3, 3)),
    ((2, 0), (2, 1), (3, 0), (3, 1), (2, 2), (2, 3), (3, 2), (3, 3)),
    ((2, 0), (2, 1), (2, 2), (2, 3)),
    ((2, 0), (2, 1), (3, 0), (3, 1), (2, 2), (2, 3), (3, 2), (3, 3)),
)


def _h(k, half):
    return tuple((k, p) for p in ((0, 1) if half == "a" else (2, 3)))


STEPS = (
    (("qk", _h(1, "a") + _h(1, "b")), ("wv",), ("gv",), ("own",),
     ("pv", _h(1, "a")), ("att", _h(3, "a")), ("c", _h(3, "a") + _h(1, "a")),
     ("pv", _h(1, "b")), ("c", _h(1, "b")),
     ("att", _h(2, "a")), ("c", _h(2, "a")), ("att", _h(3, "b")), ("c", _h(3, "b")),
     ("att", _h(2, "b")), ("c", _h(2, "b"))),
    (("qk", _h(1, "a") + _h(1, "b")), ("wv",), ("gv",),
     ("pv", _h(1, "a")), ("c", _h(1, "a")), ("pv", _h(1, "b")), ("c", _h(1, "b")),
     ("att", _h(2, "a")), ("c", _h(2, "a")), ("att", _h(3, "a")), ("c", _h(3, "a")),
     ("att", _h(3, "b")), ("c", _h(3, "b")), ("att", _h(2, "b")), ("c", _h(2, "b")), ("own",)),
    (("wv",), ("q", _h(3, "a") + _h(1, "b")), ("gv",), ("q", _h(3, "b")),
     ("att", _h(2, "a")), ("c", _h(2, "a")), ("own",), ("att", _h(2, "b")), ("c", _h(2, "b")),
     ("att", _h(1, "a")), ("c", _h(1, "a")), ("att", _h(3, "a")), ("c", _h(3, "a")),
     ("att", _h(1, "b")), ("c", _h(1, "b")), ("att", _h(3, "b")), ("c", _h(3, "b"))),
    (("qk", _h(1, "a")), ("q", _h(1, "a")), ("wv",), ("gv",),
     ("pv", _h(1, "a")), ("q", _h(1, "b")),
     ("att", _h(3, "a")), ("c", _h(3, "a")), ("att", _h(3, "b")), ("c", _h(3, "b") + _h(1, "a")),
     ("att", _h(2, "a")), ("c", _h(2, "a")), ("att", _h(2, "b")), ("c", _h(2, "b")),
     ("att", _h(1, "b")), ("c", _h(1, "b")), ("own",)),
)
OUT_ORDER = (
    ((1, 0), (1, 1), (2, 0), (3, 1), (3, 0), (2, 1)),
    ((1, 1), (1, 0), (3, 0), (2, 0), (3, 1), (2, 1)),
    ((3, 0), (3, 1), (2, 0), (1, 1), (1, 0), (2, 1)),
    ((1, 0), (3, 1), (2, 0), (1, 1), (3, 0), (2, 1)),
)


def _pack(x):
    return pltpu.bitcast(x, U32)


def _unpack(x):
    return pltpu.bitcast(x, BF16)


def _lanes(tiles):
    return jnp.concatenate([_unpack(t) for t in tiles], axis=1)


def _mod3(t):
    return jnp.where(t >= 3, t - 3, t)


def _scores(q32, ktiles):
    lane = lax.broadcasted_iota(jnp.int32, (32, 128), 1)
    zero = jnp.zeros_like(q32)
    qs = _unpack(jnp.concatenate(
        [jnp.where(lane < 64, q32, zero), jnp.where(lane >= 64, q32, zero)], axis=0))
    return jnp.dot(qs, _lanes(ktiles), preferred_element_type=F32)


def _softmax(s, last_mask):
    cols = [s[:, 128 * c:128 * (c + 1)] for c in range(s.shape[1] // 128)]
    if last_mask is not None:
        cols[-1] = jnp.where(last_mask, cols[-1], NEG)
    m = jnp.max(functools.reduce(jnp.maximum, cols), axis=1, keepdims=True)
    ps = [jnp.exp2(c - m) for c in cols]
    l = jnp.sum(functools.reduce(lambda a, b: a + b, ps), axis=1, keepdims=True)
    lane = lax.broadcasted_iota(jnp.int32, (64, 128), 1)
    inv = pl.reciprocal(jnp.where(lane < 64, l[:64], l[64:]), approx=False, full_range=False)
    return jnp.concatenate(ps, axis=1).astype(BF16), inv


def _context(p, inv, vtiles):
    lane = lax.broadcasted_iota(jnp.int32, (64, 128), 1)
    r = lax.dot_general(p, _lanes(vtiles), NT, preferred_element_type=F32)
    return _pack((jnp.where(lane < 64, r[:64], r[64:]) * inv).astype(BF16))


def _gather_sets(all_ref, set_ref):
    lo = lax.broadcasted_iota(jnp.int32, (64, 128), 1) < 64
    c = [all_ref[i] for i in range(8)]
    c0_hi = pltpu.roll(c[0], 64, 1)
    sets = (
        ((c[0], c[1]), (c[3], c[4]), (c[6], c[7])),
        ((c[1], c[2]), (c[4], c[5]), (c[7], c0_hi)),
        ((c[0], c[0]), (c[2], c[3]), (c[5], c[6])),
    )
    for r in range(3):
        for t, (a, b) in enumerate(sets[r]):
            set_ref[3 * r + t] = a if a is b else jnp.where(lo, a, b)


def _body(x_hbm, wq_hbm, kt_hbm, vt_hbm, wo_hbm, o_ref,
          kf, vf, xf, wqf, wof, wqb, wob, ksend, vsend, kall, vall, kg, vg,
          qsrc, qin, csend, cin, p_park, inv_park, all_sent,
          ld_sem, send_sem, kr_sem, vr_sem, qr_sem, cr_sem, ready):
    me = lax.axis_index("i")
    b0 = me >> 1
    hp0 = me & 1
    me3 = jnp.where(me == 3, 0, me)
    odd = hp0 == 1

    def per_chip(vals):
        if len(set(vals)) == 1:
            return vals[0]
        return jnp.where(me == 0, vals[0],
                         jnp.where(me == 1, vals[1], jnp.where(me == 2, vals[2], vals[3])))

    def on_chip(fns):
        for d in (2, 3, 1, 0):
            if fns[d] is not None:
                pl.when(me == d)(fns[d])

    def load(src, dst, i):
        return pltpu.make_async_copy(src, dst, ld_sem.at[i])

    def k_load(k):
        return load(kt_hbm.at[me ^ k], kf.at[k], k)

    def v_load(k):
        return load(vt_hbm.at[me ^ k], vf.at[k], 4 + k)

    xa_load = load(x_hbm.at[b0], xf.at[0], 8)
    xb_load = load(x_hbm.at[b0 ^ 1], xf.at[1], 9)
    wq_load = load(wq_hbm, wqf, 10)
    wo_load = load(wo_hbm, wof, 11)

    ka = jnp.where(me == 1, 1, 3)
    kb = 4 - ka

    def notify(sem, dev):
        pl.semaphore_signal(sem, inc=1, device_id=(dev,), device_id_type=MESH)

    bar = pltpu.get_barrier_semaphore()

    @pl.when(me == 0)
    def _():
        notify(bar, 1)
        notify(bar, 3)

    k_load(ka).start()

    @pl.when(me == 2)
    def _():
        pl.semaphore_wait(bar, 2)
        notify(ready.at[2], 1)
        notify(ready.at[0], 3)
        notify(ready.at[1], 0)

    @pl.when(odd)
    def _():
        pl.semaphore_wait(bar, 1)
        notify(bar, 2)
        notify(ready.at[ka - 1], 0)
        v_load(ka).start()
        k_load(kb).start()

    @pl.when(jnp.logical_not(odd))
    def _():
        k_load(kb).start()
        v_load(ka).start()

    v_load(kb).start()

    def remote(src, dst, recv_sem, k):
        return pltpu.make_async_remote_copy(
            src_ref=src, dst_ref=dst, send_sem=send_sem, recv_sem=recv_sem,
            device_id=(me ^ k,), device_id_type=MESH)

    def kv_copy(send, full, sem, k, src_chip):
        return remote(send.at[k - 1], full.at[pl.ds(2 * src_chip, 2)], sem.at[k - 1], k)

    def q_copy(k, p):
        rows = pl.ds(32 * p, 32)
        return remote(qsrc.at[k, rows], qin.at[k - 1, rows], qr_sem.at[4 * (k - 1) + p], k)

    def c_copy(k, p):
        rows = pl.ds(pl.multiple_of(32 * p, 32), 32)
        return remote(csend.at[k - 1, rows], cin.at[k, rows], cr_sem.at[4 * (k - 1) + p], k)

    def start_q(blocks):
        for k, p in blocks:
            q_copy(k, p).start()

    def start_q_per_chip(table):
        on_chip([functools.partial(start_q, t) if t else None for t in table])

    def cast(ld, src, k, dst):
        ld.wait()
        dst[0] = _pack(src[k, :, 0:128].astype(BF16))
        dst[1] = _pack(src[k, :, 128:256].astype(BF16))

    def send_k(k, needs_ready):
        cast(k_load(k), kf, k, ksend.at[k - 1])

        @pl.when(needs_ready)
        def _():
            pl.semaphore_wait(ready.at[k - 1], 1)
        kv_copy(ksend, kall, kr_sem, k, me).start()

    def send_v(k):
        cast(v_load(k), vf, k, vsend.at[k - 1])
        kv_copy(vsend, vall, vr_sem, k, me).start()

    def q_proj(half):
        q = jnp.dot(xf[half].astype(BF16), wqb[...], preferred_element_type=F32)
        q = (q * QSCALE).astype(BF16)
        for i in range(4):
            off = pl.multiple_of(32 * _mod3(i + me3), 32) if i < 3 else 96
            for hp in range(2):
                qsrc[2 * half + (hp ^ hp0), pl.ds(off, 32), :] = _pack(
                    q[64 * i:64 * (i + 1), 128 * hp:128 * (hp + 1)])

    send_k(ka, me == 0)
    for cp in (wq_load, xa_load, k_load(2), xb_load, v_load(2), k_load(0), v_load(0), wo_load):
        cp.start()

    @pl.when(odd)
    def _():
        send_v(ka)
        send_k(kb, me != 2)

    @pl.when(jnp.logical_not(odd))
    def _():
        send_k(kb, me != 2)
        send_v(ka)

    send_v(kb)
    wq_load.wait()
    wqb[...] = wqf[...].astype(BF16)
    xa_load.wait()
    q_proj(0)
    start_q_per_chip(EARLY_Q)
    send_k(2, me == 0)
    xb_load.wait()
    q_proj(1)
    send_v(2)
    start_q_per_chip(LINK_Q)
    cast(k_load(0), kf, 0, kall.at[pl.ds(2 * me, 2)])
    cast(v_load(0), vf, 0, vall.at[pl.ds(2 * me, 2)])
    wo_load.wait()
    for j, hp in enumerate((hp0, hp0 ^ 1)):
        for t in range(4):
            wob[4 * j + t] = _pack(wof[hp, :, 128 * t:128 * (t + 1)].astype(BF16))
    o_ref[b0 ^ 1] = jnp.zeros((256, 512), F32)

    lane128 = lax.broadcasted_iota(jnp.int32, (128, 128), 1)

    def block(k, p):
        s = me ^ k
        s3 = jnp.where(s == 3, 0, s)
        r, i = (p, _mod3(p + 3 - s3)) if p < 3 else (s3, 3)
        return r, i, 2 * s + (i >> 1)

    def tiles(sets, full, k, p):
        r, _, c = block(k, p)
        return [sets[3 * r + t] for t in range(3)] + ([full[c]] if p != 0 else [])

    def scores(k, p):
        src = qsrc.at[0] if k == 0 else qin.at[k - 1]
        return _scores(src[pl.ds(32 * p, 32), :], tiles(kg, kall, k, p))

    def softmax(k, p, s):
        if p == 0:
            return _softmax(s, None)
        r, i, _ = block(k, p)
        keep = (lane128 >= 64) == ((i & 1) == 1)
        if p == 3:
            keep = jnp.logical_and(keep, r != 0)
        return _softmax(s, keep)

    def context(k, p, prob, inv):
        dst = cin.at[0] if k == 0 else csend.at[k - 1]
        dst[pl.ds(32 * p, 32), :] = _context(prob, inv, tiles(vg, vall, k, p))

    def wait_q(blocks):
        for k, p in blocks:
            q_copy(k, p).wait_recv()

    def attend(blocks):
        wait_q(blocks)
        s = scores(*blocks[0])
        for n, blk in enumerate(blocks):
            nxt = scores(*blocks[n + 1]) if n + 1 < len(blocks) else None
            context(*blk, *softmax(*blk, s))
            s = nxt

    def park(blocks):
        for k, p in blocks:
            prob, inv = softmax(k, p, scores(k, p))
            packed = _pack(prob)
            for t in range(prob.shape[1] // 128):
                p_park[16 * k + 4 * p + t] = packed[:, 128 * t:128 * (t + 1)]
            inv_park[4 * k + p] = inv

    def unpark(blocks):
        for k, p in blocks:
            prob = _lanes([p_park[16 * k + 4 * p + t] for t in range(3 if p == 0 else 4)])
            context(k, p, prob, inv_park[4 * k + p])

    def out_rows(p):
        i = jnp.where(p == 3, 3, _mod3(jnp.minimum(p, 2) + 3 - me3))
        return pl.ds(pl.multiple_of(64 * i, 64), 64)

    def wo_half(j):
        return _lanes([wob[4 * j + t] for t in range(4)])

    own = [(0, p) for p in range(4)]

    def run(steps):
        for op, *arg in steps:
            if op == "qk":
                wait_q(arg[0])
                park(arg[0])
            elif op == "wv":
                for k in (3, 1, 2):
                    kv_copy(vsend, vall, vr_sem, k, me ^ k).wait_recv()
            elif op == "gv":
                _gather_sets(vall, vg)
            elif op == "pv":
                unpark(arg[0])
            elif op == "att":
                attend(arg[0])
            elif op == "c":
                for k, p in arg[0]:
                    c_copy(k, p).start()
            elif op == "q":
                start_q(arg[0])
            else:
                unpark(own)
                y = jnp.dot(_unpack(cin[0]), wo_half(0), preferred_element_type=F32)
                for p in range(4):
                    o_ref[b0, out_rows(p), :] = y[64 * p:64 * (p + 1)]

    for k in (3, 1, 2):
        kv_copy(ksend, kall, kr_sem, k, me ^ k).wait_recv()
    _gather_sets(kall, kg)
    park(own)
    on_chip([functools.partial(run, s) for s in STEPS])

    for n in range(6):
        k = per_chip([o[n][0] for o in OUT_ORDER])
        h = per_chip([o[n][1] for o in OUT_ORDER])
        b = jnp.where(k < 2, b0, b0 ^ 1)
        w = wo_half(k & 1)
        if n < 5:
            c_copy(k, 2 * h).wait_recv()
            c_copy(k, 2 * h + 1).wait_recv()
            ctx = _unpack(cin[k, pl.ds(pl.multiple_of(64 * h, 64), 64), :])
            y = jnp.dot(ctx, w, preferred_element_type=F32)
            for j in range(2):
                rows = out_rows(2 * h + j)
                o_ref[b, rows, :] = o_ref[b, rows, :] + y[64 * j:64 * (j + 1)]
        else:
            for j in range(2):
                p = 2 * h + j
                rows = out_rows(p)
                old = o_ref[b, rows, :]
                c_copy(k, p).wait_recv()
                ctx = _unpack(cin[k, pl.ds(pl.multiple_of(32 * p, 32), 32), :])
                o_ref[b, rows, :] = old + jnp.dot(ctx, w, preferred_element_type=F32)

    pltpu.make_async_copy(all_sent, all_sent, send_sem).wait()


def pallas_dist_sparse_attn_blocksparse_qseq_kvseq_b2_sq256_skv256_hq4_dh64_kernel(
    x: jax.Array,
    Wq: jax.Array,
    K_ext: jax.Array,
    V_ext: jax.Array,
    Wo: jax.Array,
):
    kt = jnp.transpose(K_ext, (0, 2, 3, 1)).reshape(4, 128, 256)
    vt = jnp.transpose(V_ext, (0, 2, 3, 1)).reshape(4, 128, 256)
    hbm = pl.BlockSpec(memory_space=pl.ANY)
    dma = pltpu.SemaphoreType.DMA
    return pl.pallas_call(
        _body,
        out_shape=jax.ShapeDtypeStruct((2, 256, 512), F32),
        in_specs=[hbm] * 5,
        out_specs=pl.BlockSpec(memory_space=pltpu.VMEM),
        scratch_shapes=[
            pltpu.VMEM((4, 128, 256), F32),
            pltpu.VMEM((4, 128, 256), F32),
            pltpu.VMEM((2, 256, 512), F32),
            pltpu.VMEM((512, 256), F32),
            pltpu.VMEM((2, 128, 512), F32),
            pltpu.VMEM((512, 256), BF16),
            pltpu.VMEM((8, 64, 128), U32),
            pltpu.VMEM((3, 2, 64, 128), U32),
            pltpu.VMEM((3, 2, 64, 128), U32),
            pltpu.VMEM((8, 64, 128), U32),
            pltpu.VMEM((8, 64, 128), U32),
            pltpu.VMEM((9, 64, 128), U32),
            pltpu.VMEM((9, 64, 128), U32),
            pltpu.VMEM((4, 128, 128), U32),
            pltpu.VMEM((3, 128, 128), U32),
            pltpu.VMEM((3, 128, 128), U32),
            pltpu.VMEM((4, 128, 128), U32),
            pltpu.VMEM((32, 64, 128), U32),
            pltpu.VMEM((8, 64, 128), F32),
            pltpu.VMEM((1536, 128), U32),
            dma((12,)), dma(()), dma((3,)), dma((3,)), dma((12,)), dma((12,)),
            pltpu.SemaphoreType.REGULAR((3,)),
        ],
        compiler_params=pltpu.CompilerParams(
            collective_id=0,
            vmem_limit_bytes=64 * 1024 * 1024,
            disable_bounds_checks=True,
            disable_semaphore_checks=True,
        ),
    )(x, Wq, kt, vt, Wo.reshape(2, 128, 512))
```
